```python
import numpy as np

kernel_name = "dist_rope_attn_qseq_b2_sq128_d512_hq4_dh64"

def setup_inputs():
    x = np.random.randn(2, 512, 512).astype(np.float32)
    Wq = np.random.randn(512, 256).astype(np.float32) * 0.02
    Wk = np.random.randn(512, 256).astype(np.float32) * 0.02
    Wv = np.random.randn(512, 256).astype(np.float32) * 0.02
    Wo = np.random.randn(256, 512).astype(np.float32) * 0.02
    return {"x": x, "Wq": Wq, "Wk": Wk, "Wv": Wv, "Wo": Wo}

def reference(x, Wq, Wk, Wv, Wo):
    B, Sq, Hq, Dh = 2, 512, 4, 64
    inv = 1.0 / (10000.0 ** (np.arange(0, Dh, 2) / Dh))
    pos = np.arange(Sq)[:, None] * inv[None, :]
    cos = np.repeat(np.cos(pos), 2, axis=-1).astype(np.float32)
    sin = np.repeat(np.sin(pos), 2, axis=-1).astype(np.float32)
    def rot(t):
        t2 = t.reshape(B, Sq, Hq, Dh // 2, 2)
        t_r = np.stack([-t2[..., 1], t2[..., 0]], axis=-1).reshape(B, Sq, Hq, Dh)
        return t * cos[None, :, None, :] + t_r * sin[None, :, None, :]
    Q = rot((x @ Wq).reshape(B, Sq, Hq, Dh))
    K = rot((x @ Wk).reshape(B, Sq, Hq, Dh))
    V = (x @ Wv).reshape(B, Sq, Hq, Dh)
    s = np.einsum('bihd,bjhd->bhij', Q, K).astype(np.float32) * 0.125
    s_max = s.max(axis=-1, keepdims=True)
    w = np.exp(s - s_max)
    w = w / w.sum(axis=-1, keepdims=True)
    ctx = np.einsum('bhij,bjhd->bihd', w, V).reshape(B, Sq, Hq * Dh)
    return ctx @ Wo
```

```python
import jax
import jax.numpy as jnp
from jax import lax
from jax.experimental import pallas as pl
from jax.experimental.pallas import tpu as pltpu

N_DEV = 4
SQ_L = 128
D = 512
HD = 256
DH = 64


def pallas_dist_rope_attn_qseq_b2_sq128_d512_hq4_dh64_kernel(
    x: jax.Array,
    Wq: jax.Array,
    Wk: jax.Array,
    Wv: jax.Array,
    Wo: jax.Array,
):
    def body(
        x_ref, wq_ref, wk_ref, wv_ref, wo_ref, out_ref,
        send_qkv, recv_qkv, ctx_send, ctx_recv,
        send_qkv_sem, recv_qkv_sem, send_ctx_sem, recv_ctx_sem,
    ):
        my = lax.axis_index("i")

        barrier = pltpu.get_barrier_semaphore()
        for k in range(1, N_DEV):
            pl.semaphore_signal(
                barrier, inc=1, device_id=((my + k) % N_DEV,),
                device_id_type=pl.DeviceIdType.MESH,
            )
        pl.semaphore_wait(barrier, N_DEV - 1)

        row = lax.broadcasted_iota(jnp.int32, (SQ_L, 128), 0)
        lane = lax.broadcasted_iota(jnp.int32, (SQ_L, 128), 1)
        pos = (my * SQ_L + row).astype(jnp.float32)
        freq_idx = ((lane % DH) // 2).astype(jnp.float32)
        inv = jnp.exp(freq_idx * (-jnp.log(10000.0) * 2.0 / DH))
        ang = pos * inv
        cos_t = jnp.cos(ang)
        sin_t = jnp.sin(ang)
        even = (lane % 2) == 0
        sin_signed = jnp.where(even, -sin_t, sin_t)

        def rope(t):
            up = pltpu.roll(t, 127, 1)
            down = pltpu.roll(t, 1, 1)
            return t * cos_t + jnp.where(even, up, down) * sin_signed

        xb = []
        for b in range(2):
            xb.append(x_ref[b].astype(jnp.bfloat16))
        for j in range(N_DEV):
            bj, cj = j // 2, 128 * (j % 2)
            xs = xb[bj]
            q = jnp.dot(xs, wq_ref[:, cj:cj + 128].astype(jnp.bfloat16),
                        preferred_element_type=jnp.float32)
            kk = jnp.dot(xs, wk_ref[:, cj:cj + 128].astype(jnp.bfloat16),
                         preferred_element_type=jnp.float32)
            v = jnp.dot(xs, wv_ref[:, cj:cj + 128].astype(jnp.bfloat16),
                        preferred_element_type=jnp.float32)
            q = rope(q) * 0.125
            kk = rope(kk)
            tile = jnp.concatenate([q, kk, v], axis=1).astype(jnp.bfloat16)
            send_qkv[j] = tile

            @pl.when(my == j)
            def _(tile=tile, j=j):
                recv_qkv[j] = tile

        for j in range(N_DEV):
            @pl.when(my != j)
            def _(j=j):
                pltpu.make_async_remote_copy(
                    src_ref=send_qkv.at[j], dst_ref=recv_qkv.at[my],
                    send_sem=send_qkv_sem.at[j], recv_sem=recv_qkv_sem.at[my],
                    device_id=(j,), device_id_type=pl.DeviceIdType.MESH,
                ).start()
        for s in range(N_DEV):
            @pl.when(my != s)
            def _(s=s):
                pltpu.make_async_remote_copy(
                    src_ref=send_qkv.at[s], dst_ref=recv_qkv.at[s],
                    send_sem=send_qkv_sem.at[s], recv_sem=recv_qkv_sem.at[s],
                    device_id=(s,), device_id_type=pl.DeviceIdType.MESH,
                ).wait_recv()
        for j in range(N_DEV):
            @pl.when(my != j)
            def _(j=j):
                pltpu.make_async_remote_copy(
                    src_ref=send_qkv.at[j], dst_ref=recv_qkv.at[my],
                    send_sem=send_qkv_sem.at[j], recv_sem=recv_qkv_sem.at[my],
                    device_id=(j,), device_id_type=pl.DeviceIdType.MESH,
                ).wait_send()

        qa = jnp.concatenate([recv_qkv[s][:, 0:128] for s in range(N_DEV)], axis=0)
        ka = jnp.concatenate([recv_qkv[s][:, 128:256] for s in range(N_DEV)], axis=0)
        va = jnp.concatenate([recv_qkv[s][:, 256:384] for s in range(N_DEV)], axis=0)
        ctx_heads = []
        for h in range(2):
            qh = qa[:, h * DH:(h + 1) * DH]
            kh = ka[:, h * DH:(h + 1) * DH]
            vh = va[:, h * DH:(h + 1) * DH]
            s_ = lax.dot_general(qh, kh, (((1,), (1,)), ((), ())),
                                 preferred_element_type=jnp.float32)
            m = jnp.max(s_, axis=1, keepdims=True)
            p = jnp.exp(s_ - m)
            l = jnp.sum(p, axis=1, keepdims=True)
            c = jnp.dot(p.astype(jnp.bfloat16), vh,
                        preferred_element_type=jnp.float32) / l
            ctx_heads.append(c)
        ctx = jnp.concatenate(ctx_heads, axis=1).astype(jnp.bfloat16)
        for i in range(N_DEV):
            ctx_send[i] = ctx[i * SQ_L:(i + 1) * SQ_L, :]

            @pl.when(my == i)
            def _(i=i):
                ctx_recv[i] = ctx_send[i]

        for i in range(N_DEV):
            @pl.when(my != i)
            def _(i=i):
                pltpu.make_async_remote_copy(
                    src_ref=ctx_send.at[i], dst_ref=ctx_recv.at[my],
                    send_sem=send_ctx_sem.at[i], recv_sem=recv_ctx_sem.at[my],
                    device_id=(i,), device_id_type=pl.DeviceIdType.MESH,
                ).start()
        for s in range(N_DEV):
            @pl.when(my != s)
            def _(s=s):
                pltpu.make_async_remote_copy(
                    src_ref=ctx_send.at[s], dst_ref=ctx_recv.at[s],
                    send_sem=send_ctx_sem.at[s], recv_sem=recv_ctx_sem.at[s],
                    device_id=(s,), device_id_type=pl.DeviceIdType.MESH,
                ).wait_recv()
        for i in range(N_DEV):
            @pl.when(my != i)
            def _(i=i):
                pltpu.make_async_remote_copy(
                    src_ref=ctx_send.at[i], dst_ref=ctx_recv.at[my],
                    send_sem=send_ctx_sem.at[i], recv_sem=recv_ctx_sem.at[my],
                    device_id=(i,), device_id_type=pl.DeviceIdType.MESH,
                ).wait_send()

        wo_b = wo_ref[...].astype(jnp.bfloat16)
        for b in range(2):
            acc = None
            for hp in range(2):
                j = 2 * b + hp
                part = jnp.dot(ctx_recv[j], wo_b[128 * hp:128 * hp + 128, :],
                               preferred_element_type=jnp.float32)
                acc = part if acc is None else acc + part
            out_ref[b] = acc

    return pl.pallas_call(
        body,
        out_shape=jax.ShapeDtypeStruct((2, SQ_L, D), jnp.float32),
        scratch_shapes=[
            pltpu.VMEM((N_DEV, SQ_L, 384), jnp.bfloat16),
            pltpu.VMEM((N_DEV, SQ_L, 384), jnp.bfloat16),
            pltpu.VMEM((N_DEV, SQ_L, 128), jnp.bfloat16),
            pltpu.VMEM((N_DEV, SQ_L, 128), jnp.bfloat16),
            pltpu.SemaphoreType.DMA((N_DEV,)),
            pltpu.SemaphoreType.DMA((N_DEV,)),
            pltpu.SemaphoreType.DMA((N_DEV,)),
            pltpu.SemaphoreType.DMA((N_DEV,)),
        ],
        compiler_params=pltpu.CompilerParams(collective_id=0),
    )(x, Wq, Wk, Wv, Wo)
```

```python
import math

import jax
import jax.numpy as jnp
from jax import lax
from jax.experimental import pallas as pl
from jax.experimental.pallas import tpu as pltpu

N_DEV = 4
SQ_L = 128
D = 512
DH = 64
BF = jnp.bfloat16
F32 = jnp.float32


def pallas_dist_rope_attn_qseq_b2_sq128_d512_hq4_dh64_kernel(
    x: jax.Array,
    Wq: jax.Array,
    Wk: jax.Array,
    Wv: jax.Array,
    Wo: jax.Array,
):
    def body(
        x_hbm, wq_hbm, wk_hbm, wv_hbm, wo_hbm, out_hbm,
        xf, xb, wkv, wqf, wof,
        skv, rkv, sq, rq, scx, rcx, oacc,
        ld_sem, st_sem,
        kv_ssem, kv_rsem, q_ssem, q_rsem, c_ssem, c_rsem,
    ):
        me = lax.axis_index("i")
        b_me = me // 2
        c_me = me % 2
        peer = [me] + [jnp.bitwise_xor(me, e) for e in (1, 2, 3)]

        barrier = pltpu.get_barrier_semaphore()
        for e in (1, 2, 3):
            pl.semaphore_signal(barrier, inc=1, device_id=(peer[e],),
                                device_id_type=pl.DeviceIdType.MESH)

        def col(c):
            return pl.ds(pl.multiple_of(c * 128, 128), 128)

        lo = pl.ds(0, 128)
        hi = pl.ds(128, 128)
        loads = [
            (x_hbm.at[b_me], xf.at[lo]),
            (wk_hbm.at[:, col(1 - c_me)], wkv.at[1, :, lo]),
            (x_hbm.at[1 - b_me], xf.at[hi]),
            (wv_hbm.at[:, col(1 - c_me)], wkv.at[1, :, hi]),
            (wk_hbm.at[:, col(c_me)], wkv.at[0, :, lo]),
            (wv_hbm.at[:, col(c_me)], wkv.at[0, :, hi]),
            (wq_hbm.at[:, col(1 - c_me)], wqf.at[1]),
            (wq_hbm.at[:, col(c_me)], wqf.at[0]),
            (wo_hbm.at[col(c_me), :], wof.at[0]),
            (wo_hbm.at[col(1 - c_me), :], wof.at[1]),
        ]
        ld = []
        for i, (src, dst) in enumerate(loads):
            cp = pltpu.make_async_copy(src, dst, ld_sem.at[i])
            cp.start()
            ld.append(cp)

        row = lax.broadcasted_iota(jnp.int32, (SQ_L, 128), 0)
        lane = lax.broadcasted_iota(jnp.int32, (SQ_L, 128), 1)
        pos = (me * SQ_L + row).astype(F32)
        fidx = ((lane % DH) // 2).astype(F32)
        inv = jnp.exp(fidx * (-math.log(10000.0) * 2.0 / DH))
        ang = pos * inv
        cos_t = jnp.cos(ang)
        sin_t = jnp.sin(ang)
        even = (lane % 2) == 0
        sin_s = jnp.where(even, -sin_t, sin_t)
        head0 = lane < DH

        def rope(t):
            up = pltpu.roll(t, 127, 1)
            down = pltpu.roll(t, 1, 1)
            return t * cos_t + jnp.where(even, up, down) * sin_s

        def rdma(sbuf, rbuf, ssem, rsem, e):
            return pltpu.make_async_remote_copy(
                src_ref=sbuf.at[e], dst_ref=rbuf.at[e],
                send_sem=ssem.at[e], recv_sem=rsem.at[e],
                device_id=(peer[e],), device_id_type=pl.DeviceIdType.MESH)

        ld[0].wait()
        ld[2].wait()
        xb[...] = xf[...].astype(BF)

        sends = []
        barrier_waited = []

        for r in (1, 0):
            if r == 1:
                ld[1].wait(); ld[3].wait()
            else:
                ld[4].wait(); ld[5].wait()
            kv = jnp.dot(xb[...], wkv[r].astype(BF), preferred_element_type=F32)
            for h in (0, 1):
                e = r + 2 * h
                t = kv[h * 128:(h + 1) * 128]
                k = rope(t[:, :128])
                v = t[:, 128:]
                dst = rkv if e == 0 else skv
                dst[e, :, lo] = k.astype(BF)
                dst[e, :, hi] = v.astype(BF)
                if e == 0:
                    continue
                if not barrier_waited:
                    pl.semaphore_wait(barrier, 3)
                    barrier_waited.append(True)
                cp = rdma(skv, rkv, kv_ssem, kv_rsem, e)
                cp.start()
                sends.append(cp)

        for r in (1, 0):
            ld[6 if r == 1 else 7].wait()
            qq = jnp.dot(xb[...], wqf[r].astype(BF), preferred_element_type=F32)
            for h in (0, 1):
                e = r + 2 * h
                q = rope(qq[h * 128:(h + 1) * 128]) * 0.125
                if e == 0:
                    rq[0] = q.astype(BF)
                else:
                    sq[e] = q.astype(BF)
                    cp = rdma(sq, rq, q_ssem, q_rsem, e)
                    cp.start()
                    sends.append(cp)

        for e in (1, 3, 2):
            rdma(skv, rkv, kv_ssem, kv_rsem, e).wait_recv()
        k_all = rkv[:, :, lo].reshape(4 * SQ_L, 128)
        v_all = rkv[:, :, hi].reshape(4 * SQ_L, 128)

        def attend(q_bf):
            qf = q_bf.astype(F32)
            q0 = jnp.where(head0, qf, 0.0).astype(BF)
            q1 = jnp.where(head0, 0.0, qf).astype(BF)
            qcat = jnp.concatenate([q0, q1], axis=0)
            s = lax.dot_general(qcat, k_all, (((1,), (1,)), ((), ())),
                                preferred_element_type=F32)
            m = jnp.max(s, axis=1, keepdims=True)
            p = jnp.exp(s - m)
            l = jnp.sum(p, axis=1, keepdims=True)
            c = jnp.dot(p.astype(BF), v_all, preferred_element_type=F32)
            c = c / l
            return jnp.where(head0, c[:128], c[128:]).astype(BF)

        for e in (0, 1, 3, 2):
            if e != 0:
                rdma(sq, rq, q_ssem, q_rsem, e).wait_recv()
            ctx = attend(rq[e])
            if e == 0:
                rcx[0] = ctx
            else:
                scx[e] = ctx
                cp = rdma(scx, rcx, c_ssem, c_rsem, e)
                cp.start()
                sends.append(cp)

        ld[8].wait()
        ld[9].wait()
        wob = [wof[0].astype(BF), wof[1].astype(BF)]

        def proj(e):
            return jnp.dot(rcx[e], wob[e & 1], preferred_element_type=F32)

        acc0 = proj(0)
        rdma(scx, rcx, c_ssem, c_rsem, 1).wait_recv()
        oacc[0] = acc0 + proj(1)
        st0 = pltpu.make_async_copy(oacc.at[0], out_hbm.at[b_me], st_sem.at[0])
        st0.start()
        rdma(scx, rcx, c_ssem, c_rsem, 3).wait_recv()
        acc1 = proj(3)
        rdma(scx, rcx, c_ssem, c_rsem, 2).wait_recv()
        oacc[1] = acc1 + proj(2)
        st1 = pltpu.make_async_copy(oacc.at[1], out_hbm.at[1 - b_me], st_sem.at[1])
        st1.start()

        for cp in sends:
            cp.wait_send()
        st0.wait()
        st1.wait()

    any_spec = pl.BlockSpec(memory_space=pl.ANY)
    return pl.pallas_call(
        body,
        out_shape=pltpu.VMEM((2, SQ_L, D), F32),
        in_specs=[any_spec] * 5,
        out_specs=pl.BlockSpec(memory_space=pltpu.VMEM),
        scratch_shapes=[
            pltpu.VMEM((2 * SQ_L, D), F32),
            pltpu.VMEM((2 * SQ_L, D), BF),
            pltpu.VMEM((2, D, 256), F32),
            pltpu.VMEM((2, D, 128), F32),
            pltpu.VMEM((2, 128, D), F32),
            pltpu.VMEM((N_DEV, SQ_L, 256), BF),
            pltpu.VMEM((N_DEV, SQ_L, 256), BF),
            pltpu.VMEM((N_DEV, SQ_L, 128), BF),
            pltpu.VMEM((N_DEV, SQ_L, 128), BF),
            pltpu.VMEM((N_DEV, SQ_L, 128), BF),
            pltpu.VMEM((N_DEV, SQ_L, 128), BF),
            pltpu.VMEM((2, SQ_L, D), F32),
            pltpu.SemaphoreType.DMA((10,)),
            pltpu.SemaphoreType.DMA((2,)),
            pltpu.SemaphoreType.DMA((N_DEV,)),
            pltpu.SemaphoreType.DMA((N_DEV,)),
            pltpu.SemaphoreType.DMA((N_DEV,)),
            pltpu.SemaphoreType.DMA((N_DEV,)),
            pltpu.SemaphoreType.DMA((N_DEV,)),
            pltpu.SemaphoreType.DMA((N_DEV,)),
        ],
        compiler_params=pltpu.CompilerParams(collective_id=0),
    )(x, Wq, Wk, Wv, Wo)
```

```python
import math

import jax
import jax.numpy as jnp
from jax import lax
from jax.experimental import pallas as pl
from jax.experimental.pallas import tpu as pltpu

N_DEV = 4
SQ_L = 128
D = 512
DH = 64
BF = jnp.bfloat16
F32 = jnp.float32

KIND = {"q": 0, "k": 1, "v": 2, "c": 3}
WIDX = {("q", 0): 0, ("q", 1): 1, ("k", 0): 2, ("k", 1): 3, ("v", 0): 4, ("v", 1): 5}
LOADS = ("x1", "k1", "x0", "v1", "k0", "v0", "q1", "q0", "o0", "o1")
TILES = ("K3", "K1", "V3", "V1", "K2", "V2", "Q1", "Q3", "Q2", "K0", "V0", "Q0")
ATT = (1, 3, 2, 0)


def pallas_dist_rope_attn_qseq_b2_sq128_d512_hq4_dh64_kernel(
    x: jax.Array,
    Wq: jax.Array,
    Wk: jax.Array,
    Wv: jax.Array,
    Wo: jax.Array,
):
    def body(
        x_hbm, wq_hbm, wk_hbm, wv_hbm, wo_hbm, out_ref,
        xf, xb, wf, wb, wof, sbuf, rbuf,
        ld_sem, ssem, rsem,
    ):
        me = lax.axis_index("i")
        b_me = me // 2
        c_me = me % 2
        peer = [me] + [jnp.bitwise_xor(me, e) for e in (1, 2, 3)]

        barrier = pltpu.get_barrier_semaphore()
        for e in (1, 2, 3):
            pl.semaphore_signal(barrier, inc=1, device_id=(peer[e],),
                                device_id_type=pl.DeviceIdType.MESH)

        def blk(c):
            return pl.ds(pl.multiple_of(c * 128, 128), 128)

        crel = [c_me, 1 - c_me]
        w_hbm = {"q": wq_hbm, "k": wk_hbm, "v": wv_hbm}
        ld = {}
        for i, name in enumerate(LOADS):
            kind, r = name[0], int(name[1])
            if kind == "x":
                src, dst = x_hbm.at[b_me if r == 0 else 1 - b_me], xf.at[r]
            elif kind == "o":
                src, dst = wo_hbm.at[blk(crel[r]), :], wof.at[r]
            else:
                src, dst = w_hbm[kind].at[:, blk(crel[r])], wf.at[WIDX[(kind, r)]]
            cp = pltpu.make_async_copy(src, dst, ld_sem.at[i])
            cp.start()
            ld[name] = cp

        row = lax.broadcasted_iota(jnp.int32, (SQ_L, 128), 0)
        lane = lax.broadcasted_iota(jnp.int32, (SQ_L, 128), 1)
        pos = (me * SQ_L + row).astype(F32)
        fidx = ((lane % DH) // 2).astype(F32)
        inv = jnp.exp(fidx * (-math.log(10000.0) * 2.0 / DH))
        ang = pos * inv
        cos_t = jnp.cos(ang)
        sin_t = jnp.sin(ang)
        even = (lane % 2) == 0
        sin_s = jnp.where(even, -sin_t, sin_t)
        head0 = lane < DH

        def rope(t):
            up = pltpu.roll(t, 127, 1)
            down = pltpu.roll(t, 1, 1)
            return t * cos_t + jnp.where(even, up, down) * sin_s

        def rdma(kind, e):
            k = KIND[kind]
            return pltpu.make_async_remote_copy(
                src_ref=sbuf.at[k, e], dst_ref=rbuf.at[k, e],
                send_sem=ssem.at[k, e], recv_sem=rsem.at[k, e],
                device_id=(peer[e],), device_id_type=pl.DeviceIdType.MESH)

        waited, converted, barrier_waited = set(), set(), []

        def need(name):
            if name not in waited:
                ld[name].wait()
                waited.add(name)

        def xhalf(h):
            if ("x", h) not in converted:
                need(f"x{h}")
                xb[h] = xf[h].astype(BF)
                converted.add(("x", h))
            return xb[h]

        def wblock(kind, r):
            i = WIDX[(kind, r)]
            if (kind, r) not in converted:
                need(f"{kind}{r}")
                wb[i] = wf[i].astype(BF)
                converted.add((kind, r))
            return wb[i]

        sends = []

        for name in TILES:
            kind, e = name[0].lower(), int(name[1])
            h, r = e >> 1, e & 1
            t = jnp.dot(xhalf(h), wblock(kind, r), preferred_element_type=F32)
            if kind == "k":
                t = rope(t)
            elif kind == "q":
                t = rope(t) * 0.125
            if e == 0:
                rbuf[KIND[kind], 0] = t.astype(BF)
                continue
            sbuf[KIND[kind], e] = t.astype(BF)
            if not barrier_waited:
                pl.semaphore_wait(barrier, 3)
                barrier_waited.append(True)
            cp = rdma(kind, e)
            cp.start()
            sends.append(cp)

        for e in (1, 3, 2):
            rdma("k", e).wait_recv()
            rdma("v", e).wait_recv()
        k_all = rbuf[KIND["k"]].reshape(N_DEV * SQ_L, 128)
        v_all = rbuf[KIND["v"]].reshape(N_DEV * SQ_L, 128)

        def attend(q_bf):
            qf = q_bf.astype(F32)
            q0 = jnp.where(head0, qf, 0.0).astype(BF)
            q1 = jnp.where(head0, 0.0, qf).astype(BF)
            qcat = jnp.concatenate([q0, q1], axis=0)
            s = lax.dot_general(qcat, k_all, (((1,), (1,)), ((), ())),
                                preferred_element_type=F32)
            m = jnp.max(s, axis=1, keepdims=True)
            p = jnp.exp(s - m)
            l = jnp.sum(p, axis=1, keepdims=True)
            c = jnp.dot(p.astype(BF), v_all, preferred_element_type=F32)
            c = c / l
            return jnp.where(head0, c[:128], c[128:]).astype(BF)

        for e in ATT:
            if e != 0:
                rdma("q", e).wait_recv()
            ctx = attend(rbuf[KIND["q"], e])
            if e == 0:
                rbuf[KIND["c"], 0] = ctx
            else:
                sbuf[KIND["c"], e] = ctx
                cp = rdma("c", e)
                cp.start()
                sends.append(cp)

        need("o0")
        need("o1")
        wob = [wof[0].astype(BF), wof[1].astype(BF)]

        def proj(e):
            return jnp.dot(rbuf[KIND["c"], e], wob[e & 1],
                           preferred_element_type=F32)

        acc0 = proj(0)
        rdma("c", 1).wait_recv()
        out_ref[b_me] = acc0 + proj(1)
        rdma("c", 3).wait_recv()
        acc1 = proj(3)
        rdma("c", 2).wait_recv()
        out_ref[1 - b_me] = acc1 + proj(2)

        for cp in sends:
            cp.wait_send()

    any_spec = pl.BlockSpec(memory_space=pl.ANY)
    return pl.pallas_call(
        body,
        out_shape=pltpu.VMEM((2, SQ_L, D), F32),
        in_specs=[any_spec] * 5,
        out_specs=pl.BlockSpec(memory_space=pltpu.VMEM),
        scratch_shapes=[
            pltpu.VMEM((2, SQ_L, D), F32),
            pltpu.VMEM((2, SQ_L, D), BF),
            pltpu.VMEM((6, D, 128), F32),
            pltpu.VMEM((6, D, 128), BF),
            pltpu.VMEM((2, 128, D), F32),
            pltpu.VMEM((4, N_DEV, SQ_L, 128), BF),
            pltpu.VMEM((4, N_DEV, SQ_L, 128), BF),
            pltpu.SemaphoreType.DMA((len(LOADS),)),
            pltpu.SemaphoreType.DMA((4, N_DEV)),
            pltpu.SemaphoreType.DMA((4, N_DEV)),
        ],
        compiler_params=pltpu.CompilerParams(collective_id=0),
    )(x, Wq, Wk, Wv, Wo)
```
